```python
import numpy as np

kernel_name = "dist_mlpseq_tp1d_bs_rep_b64_d1024_h2048"

def setup_inputs():
    x = np.random.randn(256, 1024).astype(np.float32)
    Win0 = np.random.randn(1024, 8192).astype(np.float32)
    Wout0 = np.random.randn(8192, 1024).astype(np.float32)
    Win1 = np.random.randn(1024, 8192).astype(np.float32)
    Wout1 = np.random.randn(8192, 1024).astype(np.float32)
    Win2 = np.random.randn(1024, 8192).astype(np.float32)
    Wout2 = np.random.randn(8192, 1024).astype(np.float32)
    return {"x": x, "Win0": Win0, "Wout0": Wout0, "Win1": Win1, "Wout1": Wout1, "Win2": Win2, "Wout2": Wout2}

def reference(x, Win0, Win1, Win2, Wout0, Wout1, Wout2):
    h = x @ Win0
    h = np.maximum(h, 0.0)
    x = h @ Wout0
    h = x @ Win1
    h = np.maximum(h, 0.0)
    x = h @ Wout1
    h = x @ Win2
    h = np.maximum(h, 0.0)
    x = h @ Wout2
    return x
```

```python
import jax
import jax.numpy as jnp
from jax import lax
from jax.experimental import pallas as pl
from jax.experimental.pallas import tpu as pltpu

BF16, F32 = jnp.bfloat16, jnp.float32
N_DEV = 4
LANES = 128
N_LAYERS = 3
LAST = N_LAYERS - 1

UP_CHUNKS = ((512, 4),)
UP_CHUNKS_LAST = ((512, 3), (128, 4))
K_PIECES = (1024, 512, 512)
K_PIECES_END = (512, 512, 512, 512)
ROW_CHUNKS = 2
ROW_CHUNKS_END = 8
AHEAD = 3


def _loop(n, fn):
    lax.fori_loop(0, n, lambda i, carry: (fn(i), carry)[1], 0)


def _cols(start, size):
    return pl.ds(pl.multiple_of(start, LANES), size)


def _kernel(x_hbm, wi0, wo0, wi1, wo1, wi2, wo2, out_ref,
            wi_v, wo_v, x_v, act, h_v, acc, mine1, peer1, mine2, peer2,
            x_sem, wi_sem, wo_sem, wk_sem, ag_send, ag_recv, ar_send, ar_recv):
    wi_hbm, wo_hbm = (wi0, wi1, wi2), (wo0, wo1, wo2)
    rows_per_dev = x_hbm.shape[0]
    _, n_slabs, batch, _ = act.shape
    hidden = wi_v.shape[2]
    me = lax.axis_index("i")
    nbr = (me ^ 1, N_DEV - 1 - me)

    def remote(src, dst, send_sem, recv_sem, device):
        return pltpu.make_async_remote_copy(
            src, dst, send_sem, recv_sem,
            device_id=(device,), device_id_type=pl.DeviceIdType.MESH)

    def wi_copy(l, src, col, width, k):
        return pltpu.make_async_copy(
            src.at[:, _cols(col, width)], wi_v.at[l, :, _cols(col, width)],
            wi_sem.at[l, k])

    def wo_copy(l, src, s, rows, k0, kn, sem):
        idx = (pl.ds(k0 // 16, kn // 16), rows, _cols(s * LANES, LANES))
        return pltpu.make_async_copy(src.at[idx], wo_v.at[l].at[idx], sem)

    def tile_rows(parity):
        return pl.ds(pl.multiple_of(8 * parity, 8), 8)

    def start_wi(l):
        col = k = 0
        for width, n in UP_CHUNKS_LAST if l == LAST else UP_CHUNKS:
            _loop(n, lambda j: wi_copy(
                l, wi_hbm[l], col + j * width, width, k + j).start())
            col, k = col + width * n, k + n

    def start_wo(l):
        _loop(n_slabs, lambda s: [
            wo_copy(l, wo_hbm[l], s, tile_rows(g), 0, hidden,
                    wo_sem.at[l, s]).start() for g in range(2)])

    def start_last_slab(s, pieces):
        for i, kn in enumerate(pieces):
            _loop(2, lambda g: wo_copy(
                LAST, wo_hbm[LAST], s, tile_rows(g), sum(pieces[:i]), kn,
                wk_sem.at[s, i]).start())

    x_copy = pltpu.make_async_copy(x_hbm, x_v, x_sem)
    x_copy.start()
    start_wi(0)

    barrier = pltpu.get_barrier_semaphore()
    for p in nbr:
        pl.semaphore_signal(barrier, 1, device_id=(p,),
                            device_id_type=pl.DeviceIdType.MESH)
    x_copy.wait()

    def dev_rows(p):
        return pl.ds(pl.multiple_of(p * rows_per_dev, rows_per_dev), rows_per_dev)

    def x_half(h, p):
        return act.at[0, pl.ds(h * (n_slabs // 2), n_slabs // 2), dev_rows(p), :]

    def ag_own(j, i):
        return remote(x_half(i ^ j, me), x_half(i ^ j, me),
                      ag_send, ag_recv.at[j, i], nbr[i])

    for s in range(n_slabs):
        act[0, s, dev_rows(me), :] = x_v[:, s * LANES:(s + 1) * LANES].astype(BF16)
    pl.semaphore_wait(barrier, 2)
    _loop(2, lambda j: [ag_own(j, i).start() for i in range(2)])
    forwards = [remote(x_half(i, nbr[i]), x_half(i, nbr[i]),
                       ag_send, ag_recv.at[2, i], nbr[1 - i]) for i in range(2)]
    for i in range(2):
        ag_own(0, i).wait_recv()
        forwards[i].start()
    for copy in [ag_own(1, i) for i in range(2)] + forwards:
        copy.wait_recv()

    def up_projection(l, chunks):
        col = k = 0
        for width, n in chunks:
            def step(j):
                c = col + j * width
                wi_copy(l, wi_v.at[l], c, width, k + j).wait()
                a = jnp.concatenate([act[l, b] for b in range(n_slabs)], axis=1)
                w = wi_v[l, :, _cols(c, width)].astype(BF16)
                y = jnp.dot(a, w, preferred_element_type=F32)
                y = jnp.maximum(y, 0.0).astype(BF16)
                for b in range(width // LANES):
                    h_v[c // LANES + b] = y[:, b * LANES:(b + 1) * LANES]
            _loop(n, step)
            col, k = col + width * n, k + n

    def chunk_rows(n, c, i):
        size = batch // (2 * n)
        return pl.ds((2 * c + i) * size, size)

    def exchange(step, l, s, n, c, i):
        src, dst = ((mine1, peer1), (mine2, peer2))[step]
        r = chunk_rows(n, c, i)
        return remote(src.at[l, s, r], dst.at[l, s, r], ar_send,
                      ar_recv.at[l, s * ROW_CHUNKS + c, step, i], nbr[i ^ step])

    def down_piece(l, s, pieces, i, n, sem):
        k0, kn = sum(pieces[:i]), pieces[i]
        wo_copy(l, wo_v.at[l], s, slice(None), k0, kn, sem).wait()
        w = wo_v[l, pl.ds(k0 // 16, kn // 16), :, _cols(s * LANES, LANES)]
        h = jnp.concatenate(
            [h_v[b] for b in range(k0 // LANES, (k0 + kn) // LANES)], axis=1)
        y = jnp.dot(h, w.reshape(kn, LANES).astype(BF16),
                    preferred_element_type=F32)
        if i > 0:
            y = y + acc[...]
        if i < len(pieces) - 1:
            acc[...] = y
            return
        for c in range(n):
            for j in range(2):
                r = chunk_rows(n, c, j)
                mine1[l, s, r] = y[r.start:r.start + r.size].astype(BF16)
            for j in range(2):
                exchange(0, l, s, n, c, j).start()

    def pair_sum(l, s, n, c):
        for i in range(2):
            exchange(0, l, s, n, c, i).wait_recv()
        for i in range(2):
            r = chunk_rows(n, c, i)
            y = mine1[l, s, r].astype(F32) + peer1[l, s, r].astype(F32)
            mine2[l, s, r] = y.astype(BF16)
        for i in range(2):
            exchange(1, l, s, n, c, i).start()

    def full_sum(l, s, n, c, last):
        for i in range(2):
            exchange(1, l, s, n, c, i).wait_recv()
        for i in range(2):
            r = chunk_rows(n, c, i)
            y = mine2[l, s, r].astype(F32) + peer2[l, s, r].astype(F32)
            if last:
                out_ref[r, _cols(s * LANES, LANES)] = y.astype(out_ref.dtype)
            else:
                act[l + 1, s, r] = y.astype(BF16)

    def layer(l):
        up_projection(l, UP_CHUNKS)
        for nxt in range(1, N_LAYERS):
            pl.when(l + 1 == nxt)(lambda: start_wi(nxt))

        def slab(s):
            pl.when(s >= 2)(lambda: pair_sum(l, s - 2, 1, 0))
            down_piece(l, s, (hidden,), 0, 1, wo_sem.at[l, s])
            pl.when(s >= 4)(lambda: full_sum(l, s - 4, 1, 0, False))

        _loop(n_slabs, slab)
        for nxt in range(1, LAST):
            pl.when(l + 1 == nxt)(lambda: start_wo(nxt))
        _loop(2, lambda j: pair_sum(l, n_slabs - 2 + j, 1, 0))
        _loop(4, lambda j: full_sum(l, n_slabs - 4 + j, 1, 0, False))

    start_wo(0)
    _loop(LAST, layer)

    end, n = n_slabs - 1, ROW_CHUNKS
    _loop(AHEAD, lambda s: start_last_slab(s, K_PIECES))
    up_projection(LAST, UP_CHUNKS_LAST)

    def slab(s):
        pl.when(s + AHEAD < end)(lambda: start_last_slab(s + AHEAD, K_PIECES))
        pl.when(s + AHEAD == end)(lambda: start_last_slab(end, K_PIECES_END))
        for i in range(len(K_PIECES)):
            if i < n:
                pl.when(s >= 2)(lambda: pair_sum(LAST, s - 2, n, i))
            down_piece(LAST, s, K_PIECES, i, n, wk_sem.at[s, i])
        for c in range(n):
            pl.when(s >= 4)(lambda: full_sum(LAST, s - 4, n, c, True))

    _loop(end, slab)
    for i in range(len(K_PIECES_END)):
        if i < n:
            pair_sum(LAST, end - 2, n, i)
        down_piece(LAST, end, K_PIECES_END, i, ROW_CHUNKS_END, wk_sem.at[end, i])
    for c in range(n):
        pair_sum(LAST, end - 1, n, c)
    for s in range(end - 4, end - 1):
        for c in range(n):
            full_sum(LAST, s, n, c, True)
    for c in range(ROW_CHUNKS_END):
        pair_sum(LAST, end, ROW_CHUNKS_END, c)
    for c in range(n):
        full_sum(LAST, end - 1, n, c, True)
    for c in range(ROW_CHUNKS_END):
        full_sum(LAST, end, ROW_CHUNKS_END, c, True)

    for copy in [ag_own(j, i) for j in range(2) for i in range(2)] + forwards:
        copy.wait_send()
    for sent in (mine1, mine2):
        pltpu.make_async_copy(sent, sent, ar_send).wait()


def pallas_dist_mlpseq_tp1d_bs_rep_b64_d1024_h2048_kernel(
    x: jax.Array,
    Win0: jax.Array,
    Wout0: jax.Array,
    Win1: jax.Array,
    Wout1: jax.Array,
    Win2: jax.Array,
    Wout2: jax.Array,
):
    rows, d = x.shape
    hidden = Win0.shape[1]
    batch, n_slabs = N_DEV * rows, d // LANES
    slabs = pltpu.VMEM((N_LAYERS, n_slabs, batch, LANES), BF16)
    dma = pltpu.SemaphoreType.DMA

    def tiles(w):
        return w.reshape(hidden // 16, 16, d)

    return pl.pallas_call(
        _kernel,
        out_shape=jax.ShapeDtypeStruct((batch, d), BF16),
        in_specs=[pl.BlockSpec(memory_space=pl.ANY)] * 7,
        out_specs=pl.BlockSpec(memory_space=pltpu.VMEM),
        scratch_shapes=[
            pltpu.VMEM((N_LAYERS, d, hidden), F32),
            pltpu.VMEM((N_LAYERS, hidden // 16, 16, d), F32),
            pltpu.VMEM((rows, d), F32),
            slabs,
            pltpu.VMEM((hidden // LANES, batch, LANES), BF16),
            pltpu.VMEM((batch, LANES), F32),
            slabs, slabs, slabs, slabs,
            dma,
            dma((N_LAYERS, sum(n for _, n in UP_CHUNKS_LAST))),
            dma((LAST, n_slabs)),
            dma((n_slabs, len(K_PIECES_END))),
            dma,
            dma((3, 2)),
            dma,
            dma((N_LAYERS, (n_slabs - 1) * ROW_CHUNKS + ROW_CHUNKS_END, 2, 2)),
        ],
        compiler_params=pltpu.CompilerParams(
            vmem_limit_bytes=100 * 2**20,
            collective_id=0,
            disable_bounds_checks=True,
            disable_semaphore_checks=True,
        ),
    )(x, Win0, tiles(Wout0), Win1, tiles(Wout1), Win2, tiles(Wout2))
```

```python
import jax
import jax.numpy as jnp
from jax import lax
from jax.experimental import pallas as pl
from jax.experimental.pallas import tpu as pltpu

BF16, F32 = jnp.bfloat16, jnp.float32
N_DEV = 4
LANES = 128
N_LAYERS = 3
LAST = N_LAYERS - 1
FIRST_CHIP, REDUCER = 0, 2

UP_CHUNKS = ((512, 4),)
UP_CHUNKS_LAST = ((512, 3), (128, 4))
HEAD_START = 6
K_PIECES = (1024, 512, 512)
K_PIECES_END = (512, 512, 512, 512)
MSGS, MSGS_LAST = 2, 4
END_ROWS = 16
MIDDLE_TURN = 5
AHEAD = 3


def _loop(n, fn):
    lax.fori_loop(0, n, lambda i, carry: (fn(i), carry)[1], 0)


def _ds(start, size, align):
    if isinstance(start, int):
        return pl.ds(start, size)
    return pl.ds(pl.multiple_of(start, align), size)


def _cols(start, size):
    return _ds(start, size, LANES)


def _add(a, b):
    return a.astype(F32) + b.astype(F32)


def _kernel(x_hbm, wi0, wo0, wi1, wo1, wi2, wo2, out_ref,
            wi_v, wo_v, x_v, act, h_v, h_acc, acc, mine1, peer1, mine2, peer2,
            others, x_sem, wi_sem, wo_sem, ag_send, ag_recv, ar_send, ar_recv,
            early_send, early_recv, end_send, end_recv, hop_recv):
    wi_hbm, wo_hbm = (wi0, wi1, wi2), (wo0, wo1, wo2)
    rows_per_dev = x_hbm.shape[0]
    _, n_slabs, batch, _ = act.shape
    end = n_slabs - 1
    me = lax.axis_index("i")
    nbr = (me ^ 1, N_DEV - 1 - me)

    def remote(src, dst, send_sem, recv_sem, device):
        return pltpu.make_async_remote_copy(
            src, dst, send_sem, recv_sem,
            device_id=(device,), device_id_type=pl.DeviceIdType.MESH)

    def wait_all(ref, sem):
        pltpu.make_async_copy(ref, ref, sem).wait()

    def wi_copy(l, src, col, width, k):
        return pltpu.make_async_copy(
            src.at[:, _cols(col, width)], wi_v.at[l, :, _cols(col, width)],
            wi_sem.at[l, k])

    def wo_copy(l, src, s, pieces, i, rows=slice(None)):
        idx = (pl.ds(sum(pieces[:i]) // 16, pieces[i] // 16), rows,
               _cols(s * LANES, LANES))
        return pltpu.make_async_copy(
            src.at[idx], wo_v.at[l].at[idx], wo_sem.at[l, s, i])

    def fetch_wi(l):
        col = k = 0
        for width, n in UP_CHUNKS_LAST if l == LAST else UP_CHUNKS:
            _loop(n, lambda j: wi_copy(
                l, wi_hbm[l], col + j * width, width, k + j).start())
            col, k = col + width * n, k + n

    def fetch_slab(l, s, pieces=K_PIECES):
        for i in range(len(pieces)):
            _loop(2, lambda g: wo_copy(
                l, wo_hbm[l], s, pieces, i, _ds(8 * g, 8, 8)).start())

    x_copy = pltpu.make_async_copy(x_hbm, x_v, x_sem)
    x_copy.start()
    fetch_wi(0)

    barrier = pltpu.get_barrier_semaphore()
    for p in nbr:
        pl.semaphore_signal(barrier, 1, device_id=(p,),
                            device_id_type=pl.DeviceIdType.MESH)
    x_copy.wait()

    def dev_rows(p):
        return _ds(p * rows_per_dev, rows_per_dev, rows_per_dev)

    def x_half(h, p):
        return act.at[0, pl.ds(h * (n_slabs // 2), n_slabs // 2), dev_rows(p), :]

    def ag_own(j, i):
        return remote(x_half(i ^ j, me), x_half(i ^ j, me),
                      ag_send.at[j, i], ag_recv.at[j, i], nbr[i])

    for s in range(n_slabs):
        act[0, s, dev_rows(me), :] = x_v[:, s * LANES:(s + 1) * LANES].astype(BF16)
    pl.semaphore_wait(barrier, 2)
    _loop(2, lambda j: [ag_own(j, i).start() for i in range(2)])
    forwards = [remote(x_half(i, nbr[i]), x_half(i, nbr[i]), ag_send.at[2, i],
                       ag_recv.at[2, i], nbr[1 - i]) for i in range(2)]
    for i in range(2):
        ag_own(0, i).wait_recv()
        forwards[i].start()
    for copy in [ag_own(1, i) for i in range(2)] + forwards:
        copy.wait_recv()
    _loop(AHEAD, lambda s: fetch_slab(0, s))

    def up_dot(l, slabs, col, width):
        a = jnp.concatenate([act[l, b] for b in slabs], axis=1)
        w = wi_v[l, pl.ds(slabs[0] * LANES, len(slabs) * LANES), _cols(col, width)]
        return jnp.dot(a, w.astype(BF16), preferred_element_type=F32)

    def store_hidden(col, y):
        y = jnp.maximum(y, 0.0).astype(BF16)
        for b in range(y.shape[1] // LANES):
            h_v[col // LANES + b] = y[:, b * LANES:(b + 1) * LANES]

    def up_steps(l, chunks, col=0, k=0):
        for width, n in chunks:
            def step(j):
                c = col + j * width
                wi_copy(l, wi_v.at[l], c, width, k + j).wait()
                store_hidden(c, up_dot(l, range(n_slabs), c, width))
            _loop(n, step)
            col, k = col + width * n, k + n

    def down_dot(l, s, pieces, i, row_blocks=(slice(None),)):
        k0, kn = sum(pieces[:i]), pieces[i]
        wo_copy(l, wo_v.at[l], s, pieces, i).wait()
        w = wo_v[l, pl.ds(k0 // 16, kn // 16), :, _cols(s * LANES, LANES)]
        h = jnp.concatenate([
            jnp.concatenate([h_v[b, r] for r in row_blocks], axis=0)
            for b in range(k0 // LANES, (k0 + kn) // LANES)], axis=1)
        y = jnp.dot(h, w.reshape(kn, LANES).astype(BF16),
                    preferred_element_type=F32)
        return y + acc[...] if i > 0 else y

    def is_last(l):
        return isinstance(l, int) and l == LAST

    def msgs(l):
        return MSGS_LAST if is_last(l) else MSGS

    def exchange(step, l, s, c, i):
        src, dst = ((mine1, peer1), (mine2, peer2))[step]
        size = batch // (2 * msgs(l))
        r = pl.ds((2 * c + i) * size, size)
        sem = l * n_slabs * MSGS + s * msgs(l) + c
        return remote(src.at[l, s, r], dst.at[l, s, r],
                      ar_send.at[int(is_last(l)), step],
                      ar_recv.at[sem, step, i], nbr[i ^ step])

    def chunk(l, c):
        return pl.ds(c * (batch // msgs(l)), batch // msgs(l))

    def down(l, s, *piece_ids, pieces=K_PIECES):
        for i in piece_ids or range(len(pieces)):
            y = down_dot(l, s, pieces, i)
            if i < len(pieces) - 1:
                acc[...] = y
                continue
            for c in range(msgs(l)):
                r = chunk(l, c)
                mine1[l, s, r] = y[r.start:r.start + r.size].astype(BF16)
                for j in range(2):
                    exchange(0, l, s, c, j).start()

    def pair_sum(l, s, *chunks):
        for c in chunks or range(msgs(l)):
            for i in range(2):
                exchange(0, l, s, c, i).wait_recv()
            r = chunk(l, c)
            mine2[l, s, r] = _add(mine1[l, s, r], peer1[l, s, r]).astype(BF16)
            for i in range(2):
                exchange(1, l, s, c, i).start()

    def full_sum(l, s):
        for c in range(msgs(l)):
            for i in range(2):
                exchange(1, l, s, c, i).wait_recv()
            r = chunk(l, c)
            y = _add(mine2[l, s, r], peer2[l, s, r])
            if is_last(l):
                out_ref[r, _cols(s * LANES, LANES)] = y.astype(out_ref.dtype)
            else:
                act[l + 1, s, r] = y.astype(BF16)

    head_cols = h_acc.shape[1]

    def layer(l):
        up_steps(l, UP_CHUNKS)

        def slab(s):
            for cur in range(LAST):
                pl.when((l == cur) & (s + AHEAD <= end))(
                    lambda: fetch_slab(cur, s + AHEAD))
                pl.when((l == cur) & (s + AHEAD == end))(
                    lambda: fetch_wi(cur + 1))
            down(l, s, 0)
            pl.when(s >= 2)(lambda: pair_sum(l, s - 2))
            down(l, s, *range(1, len(K_PIECES)))
            pl.when(s >= 5)(lambda: full_sum(l, s - 5))

        _loop(n_slabs, slab)
        for nxt in range(1, LAST):
            pl.when(l + 1 == nxt)(
                lambda: _loop(AHEAD, lambda s: fetch_slab(nxt, s)))
        _loop(2, lambda j: pair_sum(l, n_slabs - 2 + j))
        _loop(HEAD_START - (n_slabs - 5), lambda j: full_sum(l, n_slabs - 5 + j))

        @pl.when(l + 1 == LAST)
        def _():
            wi_copy(LAST, wi_v.at[LAST], 0, head_cols, 0).wait()
            h_acc[...] = up_dot(LAST, range(HEAD_START), 0, head_cols)

        _loop(n_slabs - HEAD_START, lambda j: full_sum(l, HEAD_START + j))

    _loop(LAST, layer)

    is_reducer = me == REDUCER
    is_first = me == FIRST_CHIP
    pl.when(is_first)(lambda: fetch_slab(LAST, end))
    _loop(AHEAD - 1, lambda s: fetch_slab(LAST, s))
    pl.when(jnp.logical_not(is_first))(lambda: fetch_slab(LAST, AHEAD - 1))

    store_hidden(0, h_acc[...] + up_dot(
        LAST, range(HEAD_START, n_slabs), 0, head_cols))
    (width, n), *rest = UP_CHUNKS_LAST
    up_steps(LAST, [(width, n - 1)] + rest, head_cols, 1)

    side = me >> 1
    n_hops = batch // (2 * END_ROWS)

    def half(h):
        return _ds(h * (batch // 2), batch // 2, batch // 2)

    def hop_rows(h, c):
        return _ds(h * (batch // 2) + c * END_ROWS, END_ROWS, END_ROWS)

    def result(rows):
        return out_ref.at[rows, pl.ds(end * LANES, LANES)]

    def from_first(h):
        return remote(mine1.at[LAST, end, half(h)], peer1.at[LAST, end, half(h)],
                      early_send, early_recv, 1 + 2 * h)

    def to_reducer(h):
        return remote(mine1.at[LAST, end, half(h)], others.at[side, half(h)],
                      early_send, early_recv, REDUCER)

    def first_hop(h, c):
        return remote(result(hop_rows(h, c)), result(hop_rows(h, c)),
                      end_send.at[0], hop_recv.at[c], 1 + 2 * h)

    def other_half(h):
        return remote(result(half(1 - h)), result(half(1 - h)),
                      end_send.at[1], end_recv, 1 + 2 * h)

    def pieces_at(turn):
        return K_PIECES_END if turn > MIDDLE_TURN else K_PIECES

    def end_slab_early(*piece_ids):
        for i in piece_ids or range(len(K_PIECES)):
            y = down_dot(LAST, end, K_PIECES, i)
            if i < len(K_PIECES) - 1:
                acc[...] = y
            else:
                mine1[LAST, end] = y.astype(BF16)

    def drain():
        for copy in [ag_own(j, i) for j in range(2) for i in range(2)] + forwards:
            copy.wait_send()
        for step, sent in enumerate((mine1, mine2)):
            wait_all(sent.at[pl.ds(0, LAST)], ar_send.at[0, step])
            wait_all(sent.at[LAST, pl.ds(0, end)], ar_send.at[1, step])

    @pl.when(is_reducer)
    def _():
        for s in range(end):
            if s + AHEAD <= end:
                fetch_slab(LAST, s + AHEAD, pieces_at(s + AHEAD))
            down(LAST, s, pieces=pieces_at(s))
            if 1 <= s <= MIDDLE_TURN:
                pair_sum(LAST, s - 1)
        blocks = [hop_rows(h, c) for c in range(n_hops) for h in range(2)]
        for i in range(len(K_PIECES_END)):
            y = down_dot(LAST, end, K_PIECES_END, i, blocks)
            if i == len(K_PIECES_END) - 2:
                wait_all(others, early_recv)
                y = y + jnp.concatenate(
                    [_add(others[0, r], others[1, r]) for r in blocks], axis=0)
            if i < len(K_PIECES_END) - 1:
                acc[...] = y
        for k, r in enumerate(blocks):
            rows = y[k * END_ROWS:(k + 1) * END_ROWS]
            result(r)[...] = rows.astype(out_ref.dtype)
            first_hop(k % 2, k // 2).start()
        for h in range(2):
            other_half(h).start()
        for s in range(MIDDLE_TURN, end):
            pair_sum(LAST, s)
        _loop(end, lambda s: full_sum(LAST, s))
        drain()
        for k in range(2):
            wait_all(result(slice(None)), end_send.at[k])

    @pl.when((me & 1) == 1)
    def _():
        order = list(range(end))
        order.insert(MIDDLE_TURN, end)
        for turn, s in enumerate(order):
            if turn + AHEAD <= end:
                fetch_slab(LAST, order[turn + AHEAD], pieces_at(turn + AHEAD))
            if s == end:
                end_slab_early(0)
                pair_sum(LAST, turn - 2)
                end_slab_early(*range(1, len(K_PIECES)))
                to_reducer(1 - side).start()
                from_first(side).wait_recv()
                r = half(side)
                mine1[LAST, end, r] = _add(
                    mine1[LAST, end, r], peer1[LAST, end, r]).astype(BF16)
                to_reducer(side).start()
            elif turn < MIDDLE_TURN:
                down(LAST, s, 0)
                if s >= 2:
                    pair_sum(LAST, s - 2)
                down(LAST, s, *range(1, len(K_PIECES)))
            else:
                for i, chunks in enumerate(((0,), (1, 2), (3,), ())):
                    down(LAST, s, i, pieces=K_PIECES_END)
                    if chunks:
                        pair_sum(LAST, s - 1, *chunks)
        pair_sum(LAST, end - 1)
        for c in range(n_hops):
            first_hop(side, c).wait_recv()
            rows = result(hop_rows(side, c))
            remote(rows, rows, end_send.at[0], end_recv, FIRST_CHIP).start()
        _loop(end, lambda s: full_sum(LAST, s))
        drain()
        wait_all(mine1.at[LAST, end], early_send)
        wait_all(result(half(side)), end_send.at[0])
        other_half(side).wait_recv()

    @pl.when(is_first)
    def _():
        fetch_slab(LAST, AHEAD - 1)
        end_slab_early()
        for h in range(2):
            from_first(h).start()

        def slab(s):
            pl.when(s + AHEAD < end)(lambda: fetch_slab(LAST, s + AHEAD))
            down(LAST, s)
            pl.when(s >= 3)(lambda: pair_sum(LAST, s - 3))

        _loop(end, slab)
        _loop(2, lambda j: pair_sum(LAST, end - 3 + j))
        _loop(end - 3, lambda s: full_sum(LAST, s))
        pair_sum(LAST, end - 1)
        _loop(3, lambda j: full_sum(LAST, end - 3 + j))
        drain()
        wait_all(mine1.at[LAST, end], early_send)
        wait_all(result(slice(None)), end_recv)


def pallas_dist_mlpseq_tp1d_bs_rep_b64_d1024_h2048_kernel(
    x: jax.Array,
    Win0: jax.Array,
    Wout0: jax.Array,
    Win1: jax.Array,
    Wout1: jax.Array,
    Win2: jax.Array,
    Wout2: jax.Array,
):
    rows, d = x.shape
    hidden = Win0.shape[1]
    batch, n_slabs = N_DEV * rows, d // LANES
    slabs = pltpu.VMEM((N_LAYERS, n_slabs, batch, LANES), BF16)
    dma = pltpu.SemaphoreType.DMA

    def tiles(w):
        return w.reshape(hidden // 16, 16, d)

    return pl.pallas_call(
        _kernel,
        out_shape=jax.ShapeDtypeStruct((batch, d), BF16),
        in_specs=[pl.BlockSpec(memory_space=pl.ANY)] * 7,
        out_specs=pl.BlockSpec(memory_space=pltpu.VMEM),
        scratch_shapes=[
            pltpu.VMEM((N_LAYERS, d, hidden), F32),
            pltpu.VMEM((N_LAYERS, hidden // 16, 16, d), F32),
            pltpu.VMEM((rows, d), F32),
            slabs,
            pltpu.VMEM((hidden // LANES, batch, LANES), BF16),
            pltpu.VMEM((batch, UP_CHUNKS_LAST[0][0]), F32),
            pltpu.VMEM((batch, LANES), F32),
            slabs, slabs, slabs, slabs,
            pltpu.VMEM((2, batch, LANES), BF16),
            dma,
            dma((N_LAYERS, sum(n for _, n in UP_CHUNKS_LAST))),
            dma((N_LAYERS, n_slabs, len(K_PIECES_END))),
            dma((3, 2)), dma((3, 2)),
            dma((2, 2)),
            dma((LAST * n_slabs * MSGS + (n_slabs - 1) * MSGS_LAST, 2, 2)),
            dma, dma,
            dma((2,)), dma,
            dma((batch // (2 * END_ROWS),)),
        ],
        compiler_params=pltpu.CompilerParams(
            vmem_limit_bytes=100 * 2**20,
            collective_id=0,
            disable_semaphore_checks=True,
        ),
    )(x, Win0, tiles(Wout0), Win1, tiles(Wout1), Win2, tiles(Wout2))
```
